```python
import numpy as np

kernel_name = "dist_ar_xy_y_m1024_n512"

def setup_inputs():
    return {"x": np.random.randn(2048, 512).astype(np.float32)}

def reference(x: np.ndarray) -> np.ndarray:
    return x.reshape(2, 1024, 512).sum(axis=0)
```

```python
import jax
import jax.numpy as jnp
from jax import lax
from jax.experimental import pallas as pl
from jax.experimental.pallas import tpu as pltpu

MESH = pl.DeviceIdType.MESH
BLK = 16
LANES = 128
LOADS = (1, 2, 4, 7, 7, 7, 7)
TILES_PER_DMA = 2


def pallas_dist_ar_xy_y_m1024_n512_kernel(x: jax.Array):
    m, n = x.shape
    n_blk = m // BLK
    direct = sum(LOADS)
    passed = n_blk - direct
    tiles = n // LANES
    dmas = tiles // TILES_PER_DMA

    def body(x_hbm, o_ref, xv, sbuf, rbuf, lsem, ysend, yrecv, xsend, xrecv):
        mx, my = lax.axis_index("x"), lax.axis_index("y")
        y_nb, x_nb = (mx, 1 - my), (1 - mx, my)

        def row(k, count=1):
            r = jnp.where(mx == 0, k * BLK, (n_blk - k - count) * BLK)
            return pl.multiple_of(r, BLK)

        base = mx * (passed * BLK)
        loads, k = [], 0
        for j, count in enumerate(LOADS):
            r = row(k, count)
            loads.append(
                pltpu.make_async_copy(
                    x_hbm.at[pl.ds(r, count * BLK)],
                    xv.at[pl.ds(pl.multiple_of(r - base, BLK), count * BLK)],
                    lsem.at[j],
                )
            )
            k += count

        loads[0].start()
        barrier = pltpu.get_barrier_semaphore()
        for nb in (y_nb, x_nb):
            pl.semaphore_signal(barrier, 1, device_id=nb, device_id_type=MESH)
        for c in loads[1:]:
            c.start()

        def y_copy(i):
            sl = pl.ds(i * TILES_PER_DMA, TILES_PER_DMA)
            return pltpu.make_async_remote_copy(
                sbuf.at[sl], rbuf.at[sl], ysend, yrecv.at[i],
                device_id=y_nb, device_id_type=MESH,
            )

        k = 0
        for j, count in enumerate(LOADS):
            loads[j].wait()
            for kk in range(k, k + count):
                r = pl.multiple_of(row(kk) - base, BLK)
                for c in range(dmas):
                    for t in range(c * TILES_PER_DMA, (c + 1) * TILES_PER_DMA):
                        v = xv[pl.ds(r, BLK), pl.ds(t * LANES, LANES)]
                        sbuf[kk * tiles + t] = pltpu.bitcast(
                            v.astype(jnp.bfloat16), jnp.int32
                        )
                    if kk == 0 and c == 0:
                        pl.semaphore_wait(barrier, 2)
                    y_copy(kk * dmas + c).start()
            k += count

        for k in range(direct):
            r = row(k)
            for c in range(dmas):
                y_copy(k * dmas + c).wait_recv()
                for t in range(c * TILES_PER_DMA, (c + 1) * TILES_PER_DMA):
                    a = pltpu.bitcast(sbuf[k * tiles + t], jnp.bfloat16)
                    b = pltpu.bitcast(rbuf[k * tiles + t], jnp.bfloat16)
                    s = a.astype(jnp.float32) + b.astype(jnp.float32)
                    o_ref[pl.ds(r, BLK), pl.ds(t * LANES, LANES)] = s.astype(
                        jnp.bfloat16
                    )
                if k < passed:
                    width = TILES_PER_DMA * LANES
                    blk = o_ref.at[pl.ds(r, BLK), pl.ds(c * width, width)]
                    pltpu.make_async_remote_copy(
                        blk, blk, xsend, xrecv, device_id=x_nb, device_id_type=MESH
                    ).start()

        pltpu.make_async_remote_copy(
            sbuf, rbuf, ysend, yrecv.at[0], device_id=y_nb, device_id_type=MESH
        ).wait_send()
        mine = o_ref.at[pl.ds(pl.multiple_of(mx * (direct * BLK), BLK), passed * BLK)]
        theirs = o_ref.at[
            pl.ds(pl.multiple_of((1 - mx) * (direct * BLK), BLK), passed * BLK)
        ]
        pltpu.make_async_remote_copy(
            mine, theirs, xsend, xrecv, device_id=x_nb, device_id_type=MESH
        ).wait()

    return pl.pallas_call(
        body,
        out_shape=jax.ShapeDtypeStruct((m, n), jnp.bfloat16),
        in_specs=[pl.BlockSpec(memory_space=pl.ANY)],
        out_specs=pl.BlockSpec(memory_space=pltpu.VMEM),
        scratch_shapes=[
            pltpu.VMEM((direct * BLK, n), jnp.float32),
            pltpu.VMEM((direct * tiles, 8, LANES), jnp.int32),
            pltpu.VMEM((direct * tiles, 8, LANES), jnp.int32),
            pltpu.SemaphoreType.DMA((len(LOADS),)),
            pltpu.SemaphoreType.DMA,
            pltpu.SemaphoreType.DMA((direct * dmas,)),
            pltpu.SemaphoreType.DMA,
            pltpu.SemaphoreType.DMA,
        ],
        compiler_params=pltpu.CompilerParams(
            collective_id=0, disable_semaphore_checks=True
        ),
    )(x)
```

```python
import functools

import jax
import jax.numpy as jnp
import numpy as np
from jax import lax
from jax.experimental import pallas as pl
from jax.experimental.pallas import tpu as pltpu

SUBLANES, LANES = 8, 128

RING = 5
DEPTH = 9
MAX_OFFSET = 510
RADIX = 16

EXTRA = 10
HEAD = 8
MID = 4
HEAD_LOADS = (1, 1, 1, 1, 2, 2)
BARRIER_AT = 7
RELAY_AT = (0, 3, 5)
ADDS = ((0, 2, 1), (1, 2, 1))
LATE_ADDS = (4, 8)
TAIL = 8
RAW_CHUNK = 8


def _i32(v):
    return np.int32(v - (1 << 32) if v >> 31 else v)


def _each(v):
    return _i32(v * 0x01010101)


def _shl(v, k):
    if isinstance(k, int):
        return lax.shift_left(v, jnp.full_like(v, k)) if k else v
    return lax.shift_left(v, k)


def _shr(v, k):
    if isinstance(k, int):
        return lax.shift_right_logical(v, jnp.full_like(v, k)) if k else v
    return lax.shift_right_logical(v, k)


def _roll(v, k):
    return pltpu.roll(v, k % LANES, 1)


def _split(block):
    bits = block.astype(jnp.bfloat16).astype(jnp.float32)
    bits = lax.bitcast_convert_type(bits, jnp.int32)
    t = [bits[:, c * LANES : (c + 1) * LANES] for c in range(4)]
    p, q = _shr(t[0], 16) | t[1], _shr(t[2], 16) | t[3]
    keep = _i32(0x807F807F)
    kept = q & keep
    frac = (p & keep) | _shl(kept, 8) | _shr(kept, 24)
    expo = (_shr(p, 7) & _i32(0x00FF00FF)) | (_shl(q, 1) & _i32(0xFF00FF00))
    return frac, expo


def _join(frac, expo):
    keep, rest, top = _i32(0x807F807F), _i32(0x7F807F80), _i32(0xFFFF0000)
    p = (frac & keep) | (_shl(expo, 7) & rest)
    q = ((_shr(frac, 8) | _shl(frac, 24)) & keep) | (_shr(expo, 1) & rest)
    bits = jnp.concatenate([_shl(p, 16), p & top, _shl(q, 16), q & top], axis=1)
    return lax.bitcast_convert_type(bits, jnp.float32)


def _level(expos):
    even = _i32(0x00FF00FF)
    total = sum((e & even) + (_shr(e, 8) & even) for e in expos)
    total = ((total & 0xFFFF) + _shr(total, 16)).astype(jnp.float32)
    total = jnp.sum(jnp.sum(total, axis=0, keepdims=True), axis=1, keepdims=True)
    total = jnp.broadcast_to(total, (SUBLANES, LANES)).astype(jnp.int32)
    count = 4 * len(expos) * SUBLANES * LANES
    return _shr(total, count.bit_length() - 4) + 32


def _table(level):
    def each(v):
        v = v | _shl(v, 8)
        return v | _shl(v, 16)

    f = level & 7
    return (
        each(_shr(level, 3) & 255),
        each(8 - _shr(f + f + f + 2, 2)),
        each(20 - f - _shr(f, 1)),
    )


def _to_rank(expo, table):
    top, r1, r0 = table
    high = _each(0x80)
    depth = top - expo
    past1 = _shr((depth + (_each(126) - r1)) & high, 7)
    past0 = _shr((depth + (_each(127) - r0)) & high, 7)
    moved = (_each(129) - depth) & high
    odd = depth & _each(1)
    d0, d1 = r0 + _each(2), r1 + _each(1)
    step = d0 ^ ((_shl(odd, 7) - odd) & (d0 ^ d1))
    return depth, depth + past1 + past0 + ((moved - _shr(moved, 7)) & step)


def _from_rank(rank, table):
    top, r1, r0 = table
    high = _each(0x80)
    at1 = (rank + (_each(127) - r1)) & high
    past1 = (rank + (_each(126) - r1)) & high
    at0 = (rank + (_each(127) - r0)) & high
    past0 = (rank + (_each(126) - r0)) & high
    is1 = at1 ^ past1
    moved = is1 | (at0 ^ past0)
    depth = rank + _each(1) - _shr(past1, 7) - _shr(past0, 7)
    depth = (depth ^ (depth & (moved - _shr(moved, 7)))) | _shr(is1, 7)
    return top - depth


def _encode(expos, table, stream, used, bad):
    code = hi = lo = bits = wide = None
    msb = jnp.full_like(used, _i32(1 << 31))
    for j in reversed(range(4)):
        depth, rank = _to_rank(expos[j], table)
        biased = rank + _each(123)
        high = biased & _each(0x80)
        escape = _shr(high, 7)
        zeros = biased & (high - escape)
        short = _shl((biased ^ zeros) & _each(3), 2 * j)
        length = zeros + escape
        pairs = length + _shl(length, 8)
        code = short if code is None else code | short
        wide = depth | pairs if wide is None else wide | depth | pairs
        for i in (2, 0):
            first = _shr(length, 8 * i) & 31
            both = _shr(pairs, 8 * i + 8) & 31
            ones = _shr(msb, first) | _shr(msb, both)
            if hi is None:
                hi, bits = ones, both
                continue
            out = _shl(_shl(hi, 1), 31 - both)
            lo = out if lo is None else _shr(lo, both) | out
            hi = _shr(hi, both) | ones
            bits = bits + both
    bad = bad | (wide & _each(0xE0)) | (bits & ~63)
    a = used & 31
    parts = (
        _shr(hi, a),
        _shl(_shl(hi, 1), 31 - a) | _shr(lo, a),
        _shl(_shl(lo, 1), 31 - a),
    )
    at = _shr(used, 5)
    grown = []
    for k, old in enumerate(stream):
        new = jnp.zeros_like(old)
        for i, part in enumerate(parts[: k + 1]):
            new = jnp.where(at == k - i, part, new)
        grown.append(old | new)
    return code, tuple(grown), used + (bits & 63), bad


def _near_offsets(used):
    excess = ((used + 2) & ~1) - 32 * RING
    total = previous = _roll(excess, 1)
    offset = jnp.maximum(total, 0)
    for j in range(2, RADIX + 1):
        total = total + _roll(excess, j)
        offset = jnp.maximum(offset, total)
    return total, offset, previous


def _far_offsets(total, offset):
    span, best = total, offset
    for j in range(RADIX, LANES, RADIX):
        best = jnp.maximum(best, span + _roll(offset, j))
        if j + RADIX < LANES:
            span = span + _roll(total, j)
    return best


def _to_ring(stream, offset):
    a = offset & 31
    words = [_shr(stream[0], a)]
    for before, word in zip(stream, stream[1:]):
        words.append(_shr(word, a) | _shl(_shl(before, 1), 31 - a))
    words.append(_shl(_shl(stream[-1], 1), 31 - a))
    for k in (1, 2, 4, 8):
        move = (offset & (32 * k)) != 0
        pad = [jnp.zeros_like(offset)] * k
        words = [jnp.where(move, a, b) for a, b in zip(pad + words, words + pad)]
    ring = words[:RING]
    for i in range(RING, len(words)):
        ring[i % RING] = ring[i % RING] | _roll(words[i], i // RING)
    return ring


def _drop_offset(words, offset):
    for k in (8, 4, 2, 1):
        move = (offset & (32 * k)) != 0
        words = [jnp.where(move, a, b) for a, b in zip(words[k:], words)]
    a = offset & 31
    pairs = zip(words, words[1:])
    return tuple(_shl(w, a) | _shr(_shr(after, 1), 31 - a) for w, after in pairs)


def _decode(code, escapes, j, hi, lo):
    escape = _shr(escapes, 2 * j) & _each(1)
    mask = _shl(escape, 5) - escape
    zeros = used = None
    for first in (0, 2):
        left = 31
        for i in (first, first + 1):
            one = _shr(escape, 8 * i) & 1
            run = lax.clz(hi) & _shr(mask, 8 * i)
            hi = _shl(_shl(hi, one), run)
            zeros = run if i == 0 else zeros | _shl(run, 8 * i)
            left = (left - one) - run
        bits = 31 - left
        hi = hi | _shr(_shr(lo, 1), left)
        lo = _shl(lo, bits)
        used = bits if used is None else used + bits
    rank = (_shr(code, 2 * j) & _each(3)) + _shl(escape, 2) + zeros
    return rank, hi, lo, used


def _advance(stream, bits):
    moved = (*stream[1:], jnp.zeros_like(bits))
    words = [jnp.where(bits >= 32, a, b) for a, b in zip(moved, stream)]
    a = bits & 31
    pairs = zip(words, words[1:])
    return (
        *(_shl(w, a) | _shr(_shr(after, 1), 31 - a) for w, after in pairs),
        _shl(words[-1], a),
    )


def pallas_dist_ar_xy_y_m1024_n512_kernel(x: jax.Array):
    m, n = x.shape
    blocks = m // SUBLANES
    half = blocks // 2
    groups = half // 4
    ring_at = HEAD + groups + MID
    body_at = ring_at + RING
    coded = groups + RING
    y_words = half + EXTRA + coded
    x_words = half - EXTRA + coded
    span = DEPTH + 16
    raw_chunks = half // RAW_CHUNK

    def body(
        x_hbm, o_ref,
        x_vmem, out_buf, y_buf, x_buf, own_expo, ranks, raw, spill,
        out_head, y_head, x_head,
        load_sem, y_send, y_recv, x_send, x_recv, head_sem, entered, raw_sem,
    ):
        mx, my = lax.axis_index("x"), lax.axis_index("y")
        y_dev = dict(device_id=(mx, 1 - my), device_id_type=pl.DeviceIdType.MESH)
        x_dev = dict(device_id=(1 - mx, my), device_id_type=pl.DeviceIdType.MESH)

        def rows(k, count=1):
            start = (k ^ (mx * (blocks - 1))) - mx * (count - 1)
            return pl.ds(pl.multiple_of(start * SUBLANES, SUBLANES), count * SUBLANES)

        def load(k, count, i):
            r = rows(k, count)
            return pltpu.make_async_copy(x_hbm.at[r], x_vmem.at[r], load_sem.at[i])

        def slot(k):
            if isinstance(k, int):
                return k + (0 if k < HEAD else groups if k < HEAD + MID else coded)
            return k + jnp.where(k < HEAD, 0, jnp.where(k < HEAD + MID, groups, coded))

        def to_y(p):
            return pltpu.make_async_remote_copy(
                out_buf.at[p], y_buf.at[p], y_send, y_recv.at[p], **y_dev
            )

        def to_x(p):
            i = p - (body_at - 1)
            i = max(i, 0) if isinstance(p, int) else jnp.maximum(i, 0)
            return pltpu.make_async_remote_copy(
                y_buf.at[p], x_buf.at[p], x_send, x_recv.at[i], **x_dev
            )

        def relay(p):
            to_y(p).wait_recv()
            to_x(p).start()

        def add(k, frac, expo):
            r = rows(k)
            o_ref[r, :] = (x_vmem[r, :] + _join(frac, expo)).astype(o_ref.dtype)

        head_to_y = pltpu.make_async_remote_copy(
            out_head, y_head, head_sem.at[0], head_sem.at[1], **y_dev
        )
        head_to_x = pltpu.make_async_remote_copy(
            y_head, x_head, head_sem.at[2], head_sem.at[3], **x_dev
        )

        head_loads, k = {}, 0
        for i, count in enumerate(HEAD_LOADS):
            head_loads[k] = load(k, count, groups + i)
            k += count
        head_loads[0].start()
        last = jnp.logical_and(mx == 1, my == 1)
        barrier = pltpu.get_barrier_semaphore()
        pl.semaphore_signal(barrier, 1, **y_dev)
        pl.when(jnp.logical_not(last))(
            lambda: pl.semaphore_signal(barrier, 1, **x_dev)
        )
        for copy in list(head_loads.values())[1:]:
            copy.start()
        for g in range(HEAD // 4, groups):
            load(4 * g, 4, g).start()
        extra_load = load(half, EXTRA, 0)
        rest_load = load(half + EXTRA, half - EXTRA, 1)
        extra_load.start()
        rest_load.start()
        pl.when(my == 1)(lambda: pl.semaphore_wait(barrier, 1 + mx))
        pl.when(last)(lambda: pl.semaphore_signal(entered, 1, **x_dev))

        expos = []
        for k in range(HEAD):
            if k in head_loads:
                head_loads[k].wait()
            frac, expo = _split(x_vmem[rows(k), :])
            out_buf[k] = frac
            pl.when(my == 1)(to_y(k).start)
            own_expo[k] = expo
            expos.append(expo)
            if k == 3:
                level = _level(expos)
        table = _table(level)
        zero = jnp.zeros((SUBLANES, LANES), jnp.int32)
        state = ((zero,) * DEPTH, zero, zero)
        for g in range(HEAD // 4):
            code, *state = _encode(expos[4 * g : 4 * g + 4], table, *state)
            out_buf[HEAD + g] = code
            pl.when(my == 1)(to_y(HEAD + g).start)

        def encode(g, state, everyone):
            load(4 * g, 4, g).wait()
            expos = []
            for j in range(4):
                frac, expo = _split(x_vmem[rows(4 * g + j), :])
                out_buf[slot(4 * g) + j] = frac
                own_expo[4 * g + j] = expo
                expos.append(expo)
            code, *state = _encode(expos, table, *state)
            out_buf[HEAD + g] = code
            if everyone:
                to_y(HEAD + g).start()
            else:
                pl.when(my == 1)(to_y(HEAD + g).start)
            return tuple(state)

        state = lax.fori_loop(
            HEAD // 4,
            BARRIER_AT,
            functools.partial(encode, everyone=False),
            tuple(state),
        )

        @pl.when(my == 0)
        def _():
            pl.semaphore_wait(barrier, 2)
            for p in range(HEAD + BARRIER_AT):
                to_y(p).start()

        stream, used, bad = lax.fori_loop(
            BARRIER_AT, groups, functools.partial(encode, everyone=True), state
        )
        for p in range(HEAD + groups, ring_at):
            to_y(p).start()

        def early_relay(*words):
            for p in words:
                pl.when(my == 0)(functools.partial(relay, p))

        early_relay(0)
        total, offset, previous = _near_offsets(used)
        early_relay(1)
        offset = _far_offsets(total, offset)
        early_relay(2, 3)
        ring = _to_ring(stream, offset)
        early_relay(4)
        for i in range(RING):
            out_buf[ring_at + i] = ring[i]
        early_relay(5)
        for i in range(RING):
            to_y(ring_at + i).start()
        pl.when(jnp.logical_and(mx == 0, my == 1))(
            lambda: pl.semaphore_wait(entered, 1)
        )

        @pl.when(my == 1)
        def _():
            for p in range(6):
                relay(p)

        relay(6)
        fits = (
            (bad == 0)
            & (used < 32 * DEPTH)
            & (offset <= MAX_OFFSET)
            & (offset >= _roll(offset, 1) + previous)
        )
        failed = jnp.max(jnp.where(fits, 0.0, 1.0), axis=0, keepdims=True)
        relay(7)
        failed = jnp.max(failed, axis=1, keepdims=True).astype(jnp.int32)
        sublane = lax.broadcasted_iota(jnp.int32, (SUBLANES, LANES), 0)
        byte = (sublane & 6) * 4
        packed = _shl(_shr(offset, 1) & 255, byte)
        packed = packed | pltpu.roll(packed, 2, 0)
        packed = packed | pltpu.roll(packed, 4, 0)
        out_head[0] = packed[0:1]
        out_head[1] = packed[1:2]
        out_head[2] = level[:1] | _shl(jnp.broadcast_to(failed, (1, LANES)), 16)
        relay(8)
        head_to_y.start()
        extra_load.wait()
        for k in range(half, half + EXTRA):
            out_buf[slot(k)] = _split(x_vmem[rows(k), :])[0]

        r = 9
        rounds = (y_words - body_at) // 3

        @pl.loop(0, rounds)
        def _(i):
            relay(r + i)
            for j in range(3):
                to_y(body_at + 3 * i + j).start()

        for p in range(body_at + 3 * rounds, y_words):
            to_y(p).start()
        pl.loop(r + rounds, body_at)(relay)
        r = body_at

        def open_ring(head, buf, r):
            middle = (RING + span) // 2
            for i, part in enumerate((range(RING, middle), range(middle, span))):
                for w in part:
                    spill[w - RING] = _roll(buf[ring_at + w % RING], -(w // RING))
                relay(r + i)
            even, odd, info = (
                jnp.broadcast_to(head[i], (SUBLANES, LANES)) for i in range(3)
            )
            offset = jnp.where((sublane & 1) == 0, even, odd)
            offset = _shl(_shr(offset, byte) & 255, 1) + 1
            words = [buf[ring_at + w] for w in range(RING)]
            words += [spill[w] for w in range(span - RING)]
            valid = _shr(info, 16) == 0
            return _table(info & 0xFFFF), valid, _drop_offset(words, offset)

        def decoder(buf, valid, mirror, r, between):
            def step(i, stream):
                for h in range(2):
                    g = 2 * i + h
                    code = buf[HEAD + g]
                    low = _i32(0x55555555)
                    escapes = ((code | _shr(code, 1)) & low) ^ low
                    escapes = jnp.where(valid, escapes, 0)
                    hi, lo, used = stream[0], stream[1], None
                    for j in range(4):
                        if 4 * h + j in RELAY_AT:
                            c = RELAY_AT.index(4 * h + j)
                            if r is not None:
                                relay(r + len(RELAY_AT) * i + c)
                            between(i, c)
                        rank, hi, lo, bits = _decode(code, escapes, j, hi, lo)
                        used = bits if used is None else used + bits
                        ranks[(4 * g + j) ^ mirror] = rank
                    stream = _advance(stream, used)
                return stream

            return step

        def add_y(k, table):
            add(k, y_buf[slot(k)], _from_rank(ranks[k], table))

        def add_x(k):
            mine = blocks - 1 - k
            add(mine, x_buf[slot(k)], _from_rank(ranks[mine], x_table))

        def adder(done, counts):
            def between(i, c):
                for j in range(counts[c]):
                    add_y(done + sum(counts) * i + sum(counts[:c]) + j, y_table)

            return between

        steps = groups // 2
        rest_load.wait()
        relay(r)
        head_to_y.wait_recv()
        head_to_x.start()
        y_table, valid, stream = open_ring(y_head, y_buf, r + 1)
        r += 3
        lax.fori_loop(0, steps, decoder(y_buf, valid, 0, r, adder(0, ADDS[0])), stream)
        r += len(RELAY_AT) * steps
        y_done = sum(ADDS[0]) * steps

        relay(r)
        front = pl.ds(0, body_at)
        pltpu.make_async_remote_copy(
            y_buf.at[front], x_buf.at[front], x_send, x_recv.at[0], **x_dev
        ).wait_recv()
        head_to_x.wait_recv()
        x_table, valid, stream = open_ring(x_head, x_buf, r + 1)
        r += 3
        paced = (x_words - r) // len(RELAY_AT)
        step = decoder(x_buf, valid, blocks - 1, r, adder(y_done, ADDS[1]))
        stream = lax.fori_loop(0, paced, step, stream)
        for p in range(r + len(RELAY_AT) * paced, x_words):
            relay(p)
        y_done += sum(ADDS[1]) * paced

        def late_adds(i, c):
            if c:
                return
            y_count, x_count = LATE_ADDS
            y_part = [y_done + y_count * (i - paced) + j for j in range(y_count)]
            x_part = [x_count * (i - paced) + j for j in range(x_count)]
            for k in x_part:
                pl.when(k + coded >= body_at)(lambda: to_x(k + coded).wait_recv())
            for k in y_part:
                pl.when(k + coded >= x_words)(lambda: to_y(k + coded).wait_recv())
            for k in y_part:
                add_y(k, y_table)
            for k in x_part:
                add_x(k)

        step = decoder(x_buf, valid, blocks - 1, None, late_adds)
        lax.fori_loop(paced, steps, step, stream)
        y_done += LATE_ADDS[0] * (steps - paced)
        x_done = LATE_ADDS[1] * (steps - paced)

        failed = (
            _shr(out_head[2], 16)
            | _shl(_shr(y_head[2], 16), 1)
            | _shl(_shr(x_head[2], 16), 2)
        )
        failed = jnp.broadcast_to(failed, (SUBLANES, LANES))[0, 0]
        y_tail, x_tail = half + EXTRA - TAIL, half - EXTRA - TAIL
        for k in range(x_done, x_tail):
            to_x(slot(k)).wait_recv()
        for k in range(x_done, x_tail):
            add_x(k)
        for k in range(y_done, y_tail):
            if slot(k) >= x_words:
                to_y(slot(k)).wait_recv()
        for k in range(y_done, y_tail):
            add_y(k, y_table if k < half else x_table)

        def tail(i):
            ky, kx = y_tail + i, x_tail + i
            y_expo = _from_rank(ranks[ky], x_table)
            x_expo = _from_rank(ranks[blocks - 1 - kx], x_table)
            to_y(ky + coded).wait_recv()
            add(ky, y_buf[ky + coded], y_expo)
            to_x(kx + coded).wait_recv()
            add(blocks - 1 - kx, x_buf[kx + coded], x_expo)

        pl.loop(0, TAIL - 2)(tail)
        pltpu.make_async_remote_copy(
            out_buf, out_buf, y_send, y_recv.at[0], **y_dev
        ).wait_send()
        relayed = y_buf.at[pl.ds(0, x_words)]
        pltpu.make_async_remote_copy(
            relayed, relayed, x_send, x_recv.at[0], **x_dev
        ).wait_send()
        head_to_y.wait_send()
        head_to_x.wait_send()
        tail(TAIL - 2)
        tail(TAIL - 1)

        @pl.when(failed != 0)
        def _():
            def raw_to_y(c):
                part = pl.ds(c * RAW_CHUNK, RAW_CHUNK)
                return pltpu.make_async_remote_copy(
                    own_expo.at[part], raw.at[0, part],
                    raw_sem.at[0], raw_sem.at[2 + c], **y_dev,
                )

            def raw_to_x(c):
                part = pl.ds(c * RAW_CHUNK, RAW_CHUNK)
                return pltpu.make_async_remote_copy(
                    raw.at[0, part], raw.at[1, part],
                    raw_sem.at[1], raw_sem.at[2 + raw_chunks + c], **x_dev,
                )

            @pl.when((failed & 1) != 0)
            def _():
                pl.loop(0, raw_chunks)(lambda c: raw_to_y(c).start())

            @pl.when((failed & 2) != 0)
            def _():
                @pl.loop(0, raw_chunks)
                def _(c):
                    raw_to_y(c).wait_recv()
                    raw_to_x(c).start()

                pl.loop(0, half)(lambda k: add(k, y_buf[slot(k)], raw[0, k]))
                pltpu.make_async_remote_copy(
                    raw.at[0], raw.at[0], raw_sem.at[1], raw_sem.at[2], **x_dev
                ).wait_send()

            @pl.when((failed & 4) != 0)
            def _():
                pl.loop(0, raw_chunks)(lambda c: raw_to_x(c).wait_recv())

                @pl.loop(0, half - EXTRA)
                def _(k):
                    add(blocks - 1 - k, x_buf[slot(k)], raw[1, k])

                @pl.loop(half, half + EXTRA)
                def _(k):
                    add(k, y_buf[k + coded], raw[1, blocks - 1 - k])

            @pl.when((failed & 1) != 0)
            def _():
                pltpu.make_async_remote_copy(
                    own_expo, own_expo, raw_sem.at[0], raw_sem.at[2], **y_dev
                ).wait_send()

    def words(*lead):
        return pltpu.VMEM((*lead, SUBLANES, LANES), jnp.int32)

    head = pltpu.VMEM((3, 1, LANES), jnp.int32)
    dma = pltpu.SemaphoreType.DMA
    return pl.pallas_call(
        body,
        out_shape=jax.ShapeDtypeStruct((m, n), jnp.bfloat16),
        in_specs=[pl.BlockSpec(memory_space=pl.ANY)],
        out_specs=pl.BlockSpec(memory_space=pltpu.VMEM),
        scratch_shapes=[
            pltpu.VMEM((m, n), jnp.float32),
            words(y_words),
            words(y_words),
            words(x_words),
            words(half),
            words(blocks),
            words(2, half),
            words(span - RING),
            head,
            head,
            head,
            dma((groups + len(HEAD_LOADS),)),
            dma,
            dma((y_words,)),
            dma,
            dma((x_words - body_at + 1,)),
            dma((4,)),
            pltpu.SemaphoreType.REGULAR,
            dma((2 + 2 * raw_chunks,)),
        ],
        compiler_params=pltpu.CompilerParams(
            collective_id=0, disable_semaphore_checks=True
        ),
    )(x)
```

```python
import functools

import jax
import jax.numpy as jnp
import numpy as np
from jax import lax
from jax.experimental import pallas as pl
from jax.experimental.pallas import tpu as pltpu

SUBLANES, LANES = 8, 128

RING = 5
DEPTH = 9
RADIX = 16

EXTRA = 10
HEAD = 8
MID = 4
BARRIER_AT = 7
RELAY_FROM = 12
RELAY_AT = (0, 3, 5)
ADDS = ((0, 2, 1), (1, 2, 1))
LATE_ADDS = (4, 8)
LEFT = (7, 4, 2, 1, 0)
RAW_CHUNK = 8


def _i32(v):
    return np.int32(v - (1 << 32) if v >> 31 else v)


def _each(v):
    return _i32(v * 0x01010101)


def _shl(v, k):
    if isinstance(k, int):
        return lax.shift_left(v, jnp.full_like(v, k)) if k else v
    return lax.shift_left(v, k)


def _shr(v, k):
    if isinstance(k, int):
        return lax.shift_right_logical(v, jnp.full_like(v, k)) if k else v
    return lax.shift_right_logical(v, k)


def _roll(v, k):
    return pltpu.roll(v, k % LANES, 1)


def _split(block):
    bits = block.astype(jnp.bfloat16).astype(jnp.float32)
    bits = lax.bitcast_convert_type(bits, jnp.int32)
    t = [bits[:, c * LANES : (c + 1) * LANES] for c in range(4)]
    p, q = _shr(t[0], 16) | t[1], _shr(t[2], 16) | t[3]
    keep = _i32(0x807F807F)
    kept = q & keep
    frac = (p & keep) | _shl(kept, 8) | _shr(kept, 24)
    expo = (_shr(p, 7) & _i32(0x00FF00FF)) | (_shl(q, 1) & _i32(0xFF00FF00))
    return frac, expo


def _join(frac, expo):
    keep, rest, top = _i32(0x807F807F), _i32(0x7F807F80), _i32(0xFFFF0000)
    p = (frac & keep) | (_shl(expo, 7) & rest)
    q = ((_shr(frac, 8) | _shl(frac, 24)) & keep) | (_shr(expo, 1) & rest)
    bits = jnp.concatenate([_shl(p, 16), p & top, _shl(q, 16), q & top], axis=1)
    return lax.bitcast_convert_type(bits, jnp.float32)


def _level(expos):
    even = _i32(0x00FF00FF)
    total = sum((e & even) + (_shr(e, 8) & even) for e in expos)
    total = ((total & 0xFFFF) + _shr(total, 16)).astype(jnp.float32)
    total = jnp.sum(jnp.sum(total, axis=0, keepdims=True), axis=1, keepdims=True)
    total = jnp.broadcast_to(total, (SUBLANES, LANES)).astype(jnp.int32)
    count = 4 * len(expos) * SUBLANES * LANES
    return _shr(total, count.bit_length() - 4) + 32


def _table(level):
    def each(v):
        v = v | _shl(v, 8)
        return v | _shl(v, 16)

    f = level & 7
    return (
        each(_shr(level, 3) & 255),
        each(8 - _shr(f + f + f + 2, 2)),
        each(20 - f - _shr(f, 1)),
    )


def _to_rank(expo, table):
    top, r1, r0 = table
    high = _each(0x80)
    depth = top - expo
    past1 = _shr((depth + (_each(126) - r1)) & high, 7)
    past0 = _shr((depth + (_each(127) - r0)) & high, 7)
    moved = (_each(129) - depth) & high
    odd = depth & _each(1)
    d0, d1 = r0 + _each(2), r1 + _each(1)
    step = d0 ^ ((_shl(odd, 7) - odd) & (d0 ^ d1))
    return depth, depth + past1 + past0 + ((moved - _shr(moved, 7)) & step)


def _from_rank(rank, table):
    top, r1, r0 = table
    high = _each(0x80)
    at1 = (rank + (_each(127) - r1)) & high
    past1 = (rank + (_each(126) - r1)) & high
    at0 = (rank + (_each(127) - r0)) & high
    past0 = (rank + (_each(126) - r0)) & high
    is1 = at1 ^ past1
    moved = is1 | (at0 ^ past0)
    depth = rank + _each(1) - _shr(past1, 7) - _shr(past0, 7)
    depth = (depth ^ (depth & (moved - _shr(moved, 7)))) | _shr(is1, 7)
    return top - depth


def _encode(expos, table, stream, used, bad):
    code = hi = lo = bits = deep = long = None
    msb = jnp.full_like(used, _i32(1 << 31))
    for j in reversed(range(4)):
        depth, rank = _to_rank(expos[j], table)
        biased = rank + _each(123)
        high = biased & _each(0x80)
        escape = _shr(high, 7)
        zeros = biased & (high - escape)
        short = _shl((biased ^ zeros) & _each(3), 2 * j)
        length = zeros + escape
        pairs = length + _shl(length, 8)
        code = short if code is None else code | short
        deep = depth if deep is None else deep | depth
        long = pairs if long is None else long | pairs
        for i in (2, 0):
            first = _shr(length, 8 * i) & 31
            both = _shr(pairs, 8 * i + 8) & 31
            ones = _shr(msb, first) | _shr(msb, both)
            if hi is None:
                hi, bits = ones, both
                continue
            out = _shl(_shl(hi, 1), 31 - both)
            lo = out if lo is None else _shr(lo, both) | out
            hi = _shr(hi, both) | ones
            bits = bits + both
    bad = bad | (deep & _each(0xE0)) | (long & 0x60006000) | (bits & ~63)
    a = used & 31
    parts = (
        _shr(hi, a),
        _shl(_shl(hi, 1), 31 - a) | _shr(lo, a),
        _shl(_shl(lo, 1), 31 - a),
    )
    at = _shr(used, 5)
    grown = []
    for k, old in enumerate(stream):
        new = jnp.zeros_like(old)
        for i, part in enumerate(parts[: k + 1]):
            new = jnp.where(at == k - i, part, new)
        grown.append(old | new)
    return code, tuple(grown), used + (bits & 63), bad


def _near_offsets(used):
    excess = ((used + 2) & ~1) - 32 * RING
    total = previous = _roll(excess, 1)
    offset = jnp.maximum(total, 0)
    for j in range(2, RADIX + 1):
        total = total + _roll(excess, j)
        offset = jnp.maximum(offset, total)
    return total, offset, previous


def _far_offsets(total, offset):
    span, best = total, offset
    for j in range(RADIX, LANES, RADIX):
        best = jnp.maximum(best, span + _roll(offset, j))
        if j + RADIX < LANES:
            span = span + _roll(total, j)
    return best


def _to_ring(stream, offset):
    a = offset & 31
    words = [_shr(stream[0], a)]
    for before, word in zip(stream, stream[1:]):
        words.append(_shr(word, a) | _shl(_shl(before, 1), 31 - a))
    words.append(_shl(_shl(stream[-1], 1), 31 - a))
    for k in (1, 2, 4, 8):
        move = (offset & (32 * k)) != 0
        pad = [jnp.zeros_like(offset)] * k
        words = [jnp.where(move, a, b) for a, b in zip(pad + words, words + pad)]
    ring = words[:RING]
    for i in range(RING, len(words)):
        ring[i % RING] = ring[i % RING] | _roll(words[i], i // RING)
    return ring


def _drop_offset(words, offset):
    for k in (8, 4, 2, 1):
        move = (offset & (32 * k)) != 0
        words = [jnp.where(move, a, b) for a, b in zip(words[k:], words)]
    a = offset & 31
    pairs = zip(words, words[1:])
    return tuple(_shl(w, a) | _shr(_shr(after, 1), 31 - a) for w, after in pairs)


def _decode(code, escapes, j, hi, lo):
    escape = _shr(escapes, 2 * j) & _each(1)
    mask = _shl(escape, 5) - escape
    zeros = used = None
    for first in (0, 2):
        left = 31
        for i in (first, first + 1):
            one = _shr(escape, 8 * i) & 1
            run = lax.clz(hi) & _shr(mask, 8 * i)
            hi = _shl(_shl(hi, one), run)
            zeros = run if i == 0 else zeros | _shl(run, 8 * i)
            left = (left - one) - run
        bits = 31 - left
        hi = hi | _shr(_shr(lo, 1), left)
        lo = _shl(lo, bits)
        used = bits if used is None else used + bits
    rank = (_shr(code, 2 * j) & _each(3)) + _shl(escape, 2) + zeros
    return rank, hi, lo, used


def _advance(stream, bits):
    moved = (*stream[1:], jnp.zeros_like(bits))
    words = [jnp.where(bits >= 32, a, b) for a, b in zip(moved, stream)]
    a = bits & 31
    pairs = zip(words, words[1:])
    return (
        *(_shl(w, a) | _shr(_shr(after, 1), 31 - a) for w, after in pairs),
        _shl(words[-1], a),
    )


def pallas_dist_ar_xy_y_m1024_n512_kernel(x: jax.Array):
    m, n = x.shape
    blocks = m // SUBLANES
    half = blocks // 2
    groups = half // 4
    ring_at = HEAD + groups + MID
    body_at = ring_at + RING
    coded = groups + RING
    y_words = half + EXTRA + coded
    x_words = half - EXTRA + coded
    span = DEPTH + 16
    raw_chunks = half // RAW_CHUNK

    def body(
        x_hbm, o_ref,
        x_vmem, out_buf, y_buf, x_buf, own_expo, ranks, raw, spill,
        out_head, y_head, x_head,
        load_sem, y_send, y_recv, x_send, x_recv, head_sem, entered, raw_sem,
    ):
        mx, my = lax.axis_index("x"), lax.axis_index("y")
        y_dev = dict(device_id=(mx, 1 - my), device_id_type=pl.DeviceIdType.MESH)
        x_dev = dict(device_id=(1 - mx, my), device_id_type=pl.DeviceIdType.MESH)

        def rows(k, count=1):
            start = (k ^ (mx * (blocks - 1))) - mx * (count - 1)
            return pl.ds(pl.multiple_of(start * SUBLANES, SUBLANES), count * SUBLANES)

        def load(k, count, i):
            r = rows(k, count)
            return pltpu.make_async_copy(x_hbm.at[r], x_vmem.at[r], load_sem.at[i])

        def slot(k):
            if isinstance(k, int):
                return k + (0 if k < HEAD else groups if k < HEAD + MID else coded)
            return k + jnp.where(k < HEAD, 0, jnp.where(k < HEAD + MID, groups, coded))

        def to_y(p):
            return pltpu.make_async_remote_copy(
                out_buf.at[p], y_buf.at[p], y_send, y_recv.at[p], **y_dev
            )

        def to_x(p):
            i = p - (body_at - 1)
            i = max(i, 0) if isinstance(p, int) else jnp.maximum(i, 0)
            return pltpu.make_async_remote_copy(
                y_buf.at[p], x_buf.at[p], x_send, x_recv.at[i], **x_dev
            )

        def relay(p):
            to_y(p).wait_recv()
            to_x(p).start()

        def add(k, frac, expo):
            r = rows(k)
            o_ref[r, :] = (x_vmem[r, :] + _join(frac, expo)).astype(o_ref.dtype)

        head_to_y = pltpu.make_async_remote_copy(
            out_head, y_head, head_sem.at[0], head_sem.at[1], **y_dev
        )
        head_to_x = pltpu.make_async_remote_copy(
            y_head, x_head, head_sem.at[2], head_sem.at[3], **x_dev
        )

        head_loads = [load(k, 1, groups + k) for k in range(HEAD)]
        head_loads[0].start()
        last = jnp.logical_and(mx == 1, my == 1)
        barrier = pltpu.get_barrier_semaphore()
        pl.semaphore_signal(barrier, 1, **y_dev)
        pl.when(jnp.logical_not(last))(
            lambda: pl.semaphore_signal(barrier, 1, **x_dev)
        )
        for copy in head_loads[1:]:
            copy.start()
        for g in range(HEAD // 4, groups):
            load(4 * g, 4, g).start()
        extra_load = load(half, EXTRA, 0)
        rest_load = load(half + EXTRA, half - EXTRA, 1)
        extra_load.start()
        rest_load.start()
        pl.when(my == 1)(lambda: pl.semaphore_wait(barrier, 1 + mx))
        pl.when(last)(lambda: pl.semaphore_signal(entered, 1, **x_dev))

        expos = []
        for k in range(HEAD):
            head_loads[k].wait()
            frac, expo = _split(x_vmem[rows(k), :])
            out_buf[k] = frac
            pl.when(my == 1)(to_y(k).start)
            own_expo[k] = expo
            expos.append(expo)
            if k == 3:
                level = _level(expos)
        table = _table(level)
        zero = jnp.zeros((SUBLANES, LANES), jnp.int32)
        state = ((zero,) * DEPTH, zero, zero)
        for g in range(HEAD // 4):
            code, *state = _encode(expos[4 * g : 4 * g + 4], table, *state)
            out_buf[HEAD + g] = code
            pl.when(my == 1)(to_y(HEAD + g).start)

        def encode(g, state, everyone):
            if everyone:
                due = jnp.logical_and(my == 0, g >= RELAY_FROM)
                pl.when(due)(lambda: relay(g - RELAY_FROM))
            load(4 * g, 4, g).wait()
            expos = []
            for j in range(4):
                frac, expo = _split(x_vmem[rows(4 * g + j), :])
                out_buf[slot(4 * g) + j] = frac
                own_expo[4 * g + j] = expo
                expos.append(expo)
            code, *state = _encode(expos, table, *state)
            out_buf[HEAD + g] = code
            if everyone:
                to_y(HEAD + g).start()
            else:
                pl.when(my == 1)(to_y(HEAD + g).start)
            return tuple(state)

        state = lax.fori_loop(
            HEAD // 4,
            BARRIER_AT,
            functools.partial(encode, everyone=False),
            tuple(state),
        )

        @pl.when(my == 0)
        def _():
            pl.semaphore_wait(barrier, 2)
            for p in range(HEAD + BARRIER_AT):
                to_y(p).start()

        stream, used, bad = lax.fori_loop(
            BARRIER_AT, groups, functools.partial(encode, everyone=True), state
        )
        for p in range(HEAD + groups, ring_at):
            to_y(p).start()

        r = groups - RELAY_FROM

        def early_relay(r, count):
            for p in range(r, r + count):
                pl.when(my == 0)(functools.partial(relay, p))
            return r + count

        r = early_relay(r, 2)
        total, offset, previous = _near_offsets(used)
        r = early_relay(r, 2)
        offset = _far_offsets(total, offset)
        r = early_relay(r, 2)
        ring = _to_ring(stream, offset)
        r = early_relay(r, 1)
        for i in range(RING):
            out_buf[ring_at + i] = ring[i]
        r = early_relay(r, 1)
        for i in range(RING):
            to_y(ring_at + i).start()
        pl.when(jnp.logical_and(mx == 0, my == 1))(
            lambda: pl.semaphore_wait(entered, 1)
        )

        @pl.when(my == 1)
        def _():
            for p in range(r):
                relay(p)

        relay(r)
        fits = (
            (bad == 0)
            & (used < 32 * DEPTH)
            & (offset < 512)
            & (offset >= _roll(offset, 1) + previous)
        )
        own_failed = jnp.max(jnp.where(fits, 0.0, 1.0), axis=0, keepdims=True)
        relay(r + 1)
        own_failed = jnp.max(own_failed, axis=1, keepdims=True).astype(jnp.int32)
        own_failed = jnp.broadcast_to(own_failed, (SUBLANES, LANES))
        sublane = lax.broadcasted_iota(jnp.int32, (SUBLANES, LANES), 0)
        byte = (sublane & 6) * 4
        packed = _shl(_shr(offset, 1) & 255, byte)
        packed = packed | pltpu.roll(packed, 2, 0)
        packed = packed | pltpu.roll(packed, 4, 0)
        out_head[0] = packed[0:1]
        out_head[1] = packed[1:2]
        out_head[2] = (level | _shl(own_failed, 16))[0:1]
        relay(r + 2)
        head_to_y.start()
        queued = body_at + 6
        for p in range(body_at, queued):
            to_y(p).start()
        extra_load.wait()
        for k in range(half, half + EXTRA):
            out_buf[slot(k)] = _split(x_vmem[rows(k), :])[0]
        r += 3
        rounds = (y_words - queued) // 4
        assert r + rounds < body_at

        @pl.loop(0, rounds)
        def _(i):
            relay(r + i)
            for j in range(4):
                to_y(queued + 4 * i + j).start()

        for p in range(queued + 4 * rounds, y_words):
            to_y(p).start()
        pl.loop(r + rounds, body_at)(relay)
        r = body_at

        def open_ring(head, buf, r):
            middle = (RING + span) // 2
            for i, part in enumerate((range(RING, middle), range(middle, span))):
                for w in part:
                    spill[w - RING] = _roll(buf[ring_at + w % RING], -(w // RING))
                relay(r + i)
            even, odd, info = (
                jnp.broadcast_to(head[i], (SUBLANES, LANES)) for i in range(3)
            )
            offset = jnp.where((sublane & 1) == 0, even, odd)
            offset = _shl(_shr(offset, byte) & 255, 1) + 1
            words = [buf[ring_at + w] for w in range(RING)]
            words += [spill[w] for w in range(span - RING)]
            valid = _shr(info, 16) == 0
            return _table(info & 0xFFFF), valid, _drop_offset(words, offset)

        def decoder(buf, valid, mirror, r, between):
            def step(i, stream):
                for h in range(2):
                    g = 2 * i + h
                    code = buf[HEAD + g]
                    low = _i32(0x55555555)
                    escapes = ((code | _shr(code, 1)) & low) ^ low
                    escapes = jnp.where(valid, escapes, 0)
                    hi, lo, used = stream[0], stream[1], None
                    for j in range(4):
                        if 4 * h + j in RELAY_AT:
                            c = RELAY_AT.index(4 * h + j)
                            if r is not None:
                                relay(r + len(RELAY_AT) * i + c)
                            between(i, c)
                        rank, hi, lo, bits = _decode(code, escapes, j, hi, lo)
                        used = bits if used is None else used + bits
                        ranks[(4 * g + j) ^ mirror] = rank
                    stream = _advance(stream, used)
                return stream

            return step

        def add_y(k, table):
            add(k, y_buf[slot(k)], _from_rank(ranks[k], table))

        def add_x(k):
            mine = blocks - 1 - k
            add(mine, x_buf[slot(k)], _from_rank(ranks[mine], x_table))

        def adder(done, counts):
            def between(i, c):
                for j in range(counts[c]):
                    add_y(done + sum(counts) * i + sum(counts[:c]) + j, y_table)

            return between

        steps = groups // 2
        rest_load.wait()
        relay(r)
        head_to_y.wait_recv()
        head_to_x.start()
        y_table, y_valid, stream = open_ring(y_head, y_buf, r + 1)
        r += 3
        step = decoder(y_buf, y_valid, 0, r, adder(0, ADDS[0]))
        lax.fori_loop(0, steps, step, stream)
        r += len(RELAY_AT) * steps
        y_done = sum(ADDS[0]) * steps

        relay(r)
        front = x_buf.at[pl.ds(0, body_at)]
        pltpu.make_async_copy(front, front, x_recv.at[0]).wait()
        head_to_x.wait_recv()
        x_table, x_valid, stream = open_ring(x_head, x_buf, r + 1)
        r += 3
        paced = (x_words - r) // len(RELAY_AT)
        assert slot(y_done + sum(ADDS[1]) * paced) < r
        step = decoder(x_buf, x_valid, blocks - 1, r, adder(y_done, ADDS[1]))
        stream = lax.fori_loop(0, paced, step, stream)
        for p in range(r + len(RELAY_AT) * paced, x_words):
            relay(p)
        y_done += sum(ADDS[1]) * paced

        def late_adds(i, c):
            if c:
                return
            y_count, x_count = LATE_ADDS
            y_part = [y_done + y_count * (i - paced) + j for j in range(y_count)]
            x_part = [x_count * (i - paced) + j for j in range(x_count)]
            for k in x_part:
                pl.when(k + coded >= body_at)(lambda: to_x(k + coded).wait_recv())
            for k in y_part:
                pl.when(k + coded >= x_words)(lambda: to_y(k + coded).wait_recv())
            for k in y_part:
                add_y(k, y_table)
            for k in x_part:
                add_x(k)

        step = decoder(x_buf, x_valid, blocks - 1, None, late_adds)
        lax.fori_loop(paced, steps, step, stream)
        y_done += LATE_ADDS[0] * (steps - paced)
        x_done = LATE_ADDS[1] * (steps - paced)

        assert y_done <= half and body_at <= slot(x_done)
        failed = own_failed | jnp.where(y_valid, 0, 2) | jnp.where(x_valid, 0, 4)
        failed = failed[0, 0]

        def finish(y_part, x_part):
            y_expo = [
                _from_rank(ranks[k], y_table if k < half else x_table) for k in y_part
            ]
            x_expo = [_from_rank(ranks[blocks - 1 - k], x_table) for k in x_part]
            for k in y_part:
                if slot(k) >= x_words:
                    to_y(slot(k)).wait_recv()
            for k, expo in zip(y_part, y_expo):
                add(k, y_buf[slot(k)], expo)
            for k in x_part:
                to_x(slot(k)).wait_recv()
            for k, expo in zip(x_part, x_expo):
                add(blocks - 1 - k, x_buf[slot(k)], expo)

        for left in LEFT:
            if left == 0:
                pltpu.make_async_remote_copy(
                    out_buf, out_buf, y_send, y_recv.at[0], **y_dev
                ).wait_send()
                relayed = y_buf.at[pl.ds(0, x_words)]
                pltpu.make_async_remote_copy(
                    relayed, relayed, x_send, x_recv.at[0], **x_dev
                ).wait_send()
                head_to_y.wait_send()
                head_to_x.wait_send()
            y_part = range(y_done, half + EXTRA - left)
            x_part = range(x_done, half - EXTRA - left)
            for j in range(0, max(len(y_part), len(x_part)), 4):
                finish(y_part[j : j + 4], x_part[j : j + 4])
            y_done, x_done = y_part.stop, x_part.stop

        @pl.when(failed != 0)
        def _():
            def raw_to_y(c):
                part = pl.ds(c * RAW_CHUNK, RAW_CHUNK)
                return pltpu.make_async_remote_copy(
                    own_expo.at[part], raw.at[0, part],
                    raw_sem.at[0], raw_sem.at[2 + c], **y_dev,
                )

            def raw_to_x(c):
                part = pl.ds(c * RAW_CHUNK, RAW_CHUNK)
                return pltpu.make_async_remote_copy(
                    raw.at[0, part], raw.at[1, part],
                    raw_sem.at[1], raw_sem.at[2 + raw_chunks + c], **x_dev,
                )

            @pl.when((failed & 1) != 0)
            def _():
                pl.loop(0, raw_chunks)(lambda c: raw_to_y(c).start())

            @pl.when((failed & 2) != 0)
            def _():
                @pl.loop(0, raw_chunks)
                def _(c):
                    raw_to_y(c).wait_recv()
                    raw_to_x(c).start()

                pl.loop(0, half)(lambda k: add(k, y_buf[slot(k)], raw[0, k]))
                pltpu.make_async_remote_copy(
                    raw.at[0], raw.at[0], raw_sem.at[1], raw_sem.at[2], **x_dev
                ).wait_send()

            @pl.when((failed & 4) != 0)
            def _():
                pl.loop(0, raw_chunks)(lambda c: raw_to_x(c).wait_recv())

                @pl.loop(0, half - EXTRA)
                def _(k):
                    add(blocks - 1 - k, x_buf[slot(k)], raw[1, k])

                @pl.loop(half, half + EXTRA)
                def _(k):
                    add(k, y_buf[k + coded], raw[1, blocks - 1 - k])

            @pl.when((failed & 1) != 0)
            def _():
                pltpu.make_async_remote_copy(
                    own_expo, own_expo, raw_sem.at[0], raw_sem.at[2], **y_dev
                ).wait_send()

    def words(*lead):
        return pltpu.VMEM((*lead, SUBLANES, LANES), jnp.int32)

    head = pltpu.VMEM((3, 1, LANES), jnp.int32)
    dma = pltpu.SemaphoreType.DMA
    return pl.pallas_call(
        body,
        out_shape=jax.ShapeDtypeStruct((m, n), jnp.bfloat16),
        in_specs=[pl.BlockSpec(memory_space=pl.ANY)],
        out_specs=pl.BlockSpec(memory_space=pltpu.VMEM),
        scratch_shapes=[
            pltpu.VMEM((m, n), jnp.float32),
            words(y_words),
            words(y_words),
            words(x_words),
            words(half),
            words(blocks),
            words(2, half),
            words(span - RING),
            head,
            head,
            head,
            dma((groups + HEAD,)),
            dma,
            dma((y_words,)),
            dma,
            dma((x_words - body_at + 1,)),
            dma((4,)),
            pltpu.SemaphoreType.REGULAR,
            dma((2 + 2 * raw_chunks,)),
        ],
        compiler_params=pltpu.CompilerParams(
            collective_id=0, disable_semaphore_checks=True
        ),
    )(x)
```
